```python
import numpy as np

kernel_name = "dist_matmul_relu_kshard_i_m1024_n1024_k512"

def setup_inputs():
    A = np.random.randn(1024, 2048).astype(np.float32)
    B = np.random.randn(2048, 1024).astype(np.float32)
    return {"A": A, "B": B}

def reference(A: np.ndarray, B: np.ndarray) -> np.ndarray:
    z = A @ B
    return np.maximum(z, 0.0)
```

```python
import jax
import jax.numpy as jnp
from jax import lax
from jax.experimental import pallas as pl
from jax.experimental.pallas import tpu as pltpu

M, N, K = 1024, 1024, 512
R = 256
H = 128
CH = 32
NCH = H // CH
PL = 15 * 128
SIGN = 0x80008000
MAG = 0x7FFF7FFF
WR, WC = 32, 640
VT = 5
B2_GROUPS = ((0, 2), (2, 1), (3, 1))

MESH = pl.DeviceIdType.MESH
BF = jnp.bfloat16
F32 = jnp.float32
U32 = jnp.uint32

G_LOADS = (("B", 0, 128), ("A", 0, 64), ("B", 128, 128), ("A", 64, 64),
           ("B", 256, 128), ("B", 384, 128), ("B", 512, 256), ("B", 768, 256))
G_PIECES = ((0, 64, 0, 128), (0, 64, 128, 128), (64, 64, 0, 256),
            (0, 128, 256, 128), (0, 128, 384, 128), (0, 128, 512, 256),
            (0, 128, 768, 256))
W_RECT = (H - WR, WR, N - WC, WC)


def _minus_swing(rect):
    r0, nr, c0, nc = rect
    hr0, hc0 = H - WR, N - WC
    if r0 + nr <= hr0 or c0 + nc <= hc0:
        return [rect]
    out = []
    if hc0 > c0:
        out.append((r0, nr, c0, hc0 - c0))
    if hr0 > r0:
        cc = max(c0, hc0)
        out.append((r0, hr0 - r0, cc, c0 + nc - cc))
    return out


def _plan():
    g_rects = [_minus_swing(p) for p in G_PIECES]
    l_rects = [_minus_swing((0, H, c0, 512)) for c0 in (0, 512)]
    r2_rects = [_minus_swing((k * CH, CH, 0, N)) for k in range(NCH)]

    count = [0]

    def alloc(n):
        first = count[0]
        count[0] += n
        return first

    idx = dict(
        g=[alloc(len(x)) for x in g_rects],
        l=[alloc(len(x)) for x in l_rects],
        r2=[alloc(len(x)) for x in r2_rects],
        w2=alloc(2), b1=alloc(2 * NCH), b2=alloc(len(B2_GROUPS) + 1),
    )
    per_link = count[0]

    loads = []
    for ld in G_LOADS:
        if ld[0] == "B":
            loads.append(ld)
        else:
            loads += [("A", 0, h * H + ld[1], ld[2]) for h in range(2)]
    need, seen = [], set()
    for (r0, nr, c0, nc) in G_PIECES:
        mine = []
        for k, ld in enumerate(loads):
            if ld[0] == "B":
                hit = ld[1] < c0 + nc and c0 < ld[1] + ld[2]
            else:
                hit = ld[2] % H < r0 + nr and r0 < ld[2] % H + ld[3]
            if hit and k not in seen:
                mine.append(k)
                seen.add(k)
        need.append(mine)
    first_other = len(loads)
    loads += [("A", 1, H, H), ("A", 2, 0, H),
              ("A", 1, 0, H), ("A", 2, H, H),
              ("A", 3, 0, R)]
    return g_rects, l_rects, r2_rects, idx, per_link, loads, need, first_other


(G_RECTS, L_RECTS, R2_RECTS, IDX, PER_LINK, LOADS, NEED, LD_OTHER) = _plan()
I_WG = 2 * PER_LINK
I_V = I_WG + 4
NSEM = I_V + 4
assert WR == CH


def _body(a_hbm, b_hbm, out_ref,
          a_f32, b_f32, a_bf, b_bf, sg, sp, accp, accw, acco, ri, wi, ro, pk,
          in_sems, ssem, rsem):
    d = lax.axis_index("i")
    partner = (d ^ 1, 3 - d)
    region = ((d + 2) & 3, partner[0], partner[1], d)

    def grow(slot, r0):
        return pl.multiple_of(region[slot] * R + r0, 16)

    barrier = pltpu.get_barrier_semaphore()
    load_cps = []
    for k, ld in enumerate(LOADS):
        if ld[0] == "B":
            cols = pl.ds(ld[1], ld[2])
            cp = pltpu.make_async_copy(b_hbm.at[:, cols], b_f32.at[:, cols],
                                       in_sems.at[k])
        else:
            _, slot, r0, nr = ld
            cp = pltpu.make_async_copy(a_hbm.at[pl.ds(grow(slot, r0), nr)],
                                       a_f32.at[slot, pl.ds(r0, nr)],
                                       in_sems.at[k])
        cp.start()
        load_cps.append(cp)
        if k == 2:
            for p in partner:
                pl.semaphore_signal(barrier, inc=1, device_id=(p,),
                                    device_id_type=MESH)

    sends = []

    def xfer(sidx, ridx, dev, src, dst):
        return pltpu.make_async_remote_copy(
            src_ref=src, dst_ref=dst, send_sem=ssem.at[sidx],
            recv_sem=rsem.at[ridx], device_id=(dev,), device_id_type=MESH)

    def send(l, t, src, dst):
        cp = xfer(l * PER_LINK + t, l * PER_LINK + t, partner[l], src, dst)
        cp.start()
        sends.append(cp)

    def wait_sem(ridx, dst):
        xfer(0, ridx, partner[0], dst, dst).wait_recv()

    def recv(l, t, dst):
        wait_sem(l * PER_LINK + t, dst)

    def rc(ref, h, rect):
        r0, nr, c0, nc = rect
        return ref.at[pl.ds(h * H + r0, nr), pl.ds(c0, nc)]

    def mm(lhs, cols=slice(None)):
        return jnp.dot(lhs, b_bf[:, cols], preferred_element_type=F32)

    def w_rows(h):
        return pl.ds(h * H + H - WR, WR)

    w_cols = pl.ds(N - WC, WC)

    for k, (r0, nr, c0, nc) in enumerate(G_PIECES):
        for j in NEED[k]:
            load_cps[j].wait()
            ld = LOADS[j]
            if ld[0] == "B":
                cols = pl.ds(ld[1], ld[2])
                b_bf[:, cols] = b_f32[:, cols].astype(BF)
            else:
                rows = pl.ds(ld[2], ld[3])
                a_bf[rows, :] = a_f32[0, rows, :].astype(BF)
        cols = pl.ds(c0, nc)
        if nr == H:
            sg[:, cols] = mm(a_bf[...], cols).astype(BF)
        else:
            lhs = jnp.concatenate(
                [a_bf[pl.ds(r0, nr), :], a_bf[pl.ds(H + r0, nr), :]], axis=0)
            res = mm(lhs, cols).astype(BF)
            sg[pl.ds(r0, nr), cols] = res[:nr]
            sg[pl.ds(H + r0, nr), cols] = res[nr:]
        if k == 0:
            pl.semaphore_wait(barrier, 2)
        for j, rect in enumerate(G_RECTS[k]):
            for l in range(2):
                send(l, IDX["g"][k] + j, rc(sg, 1 - l, rect),
                     rc(ri.at[1 - l], 0, rect))
    for h in range(2):
        flip = d == (3 if h == 0 else 1)
        q = jnp.where(flip, 1 - h, h)
        dev = jnp.where(flip, partner[h], partner[1 - h])
        cp = xfer(I_WG + h, I_WG + 2 * q + h, dev, rc(sg, h, W_RECT),
                  wi.at[q, h])
        cp.start()
        sends.append(cp)

    load_cps[LD_OTHER].wait()
    load_cps[LD_OTHER + 1].wait()
    a_bf[pl.ds(0, H), :] = a_f32[1, pl.ds(H, H), :].astype(BF)
    a_bf[pl.ds(H, H), :] = a_f32[2, pl.ds(0, H), :].astype(BF)
    for ci in range(2):
        cols = pl.ds(ci * 512, 512)
        res = mm(a_bf[...], cols)
        for l in range(2):
            sp[l, pl.ds((1 - l) * H, H), cols] = (
                res[l * H:(l + 1) * H].astype(BF))
            accw[l, :, cols] = res[(l + 1) * H - WR:(l + 1) * H]
        for j, rect in enumerate(L_RECTS[ci]):
            for l in range(2):
                send(l, IDX["l"][ci] + j, rc(sp.at[l], 1 - l, rect),
                     rc(ro.at[l], 1 - l, rect))

    for l in range(2):
        load_cps[LD_OTHER + 2 + l].wait()
        accp[l] = mm(a_f32[1 + l, pl.ds(l * H, H), :].astype(BF))
    load_cps[LD_OTHER + 4].wait()
    for h in range(2):
        rows = pl.ds(h * H, H)
        acco[rows, :] = mm(a_f32[3, rows, :].astype(BF))

    for l in range(2):
        for k in range(len(G_PIECES)):
            for j, rect in enumerate(G_RECTS[k]):
                recv(1 - l, IDX["g"][k] + j, rc(ri.at[l], 0, rect))
        for k in range(NCH):
            for j, rect in enumerate(R2_RECTS[k]):
                r0, nr, c0, nc = rect
                rows, cols = pl.ds(r0, nr), pl.ds(c0, nc)
                sp[l, pl.ds(l * H + r0, nr), cols] = (
                    accp[l, rows, cols] + ri[l, rows, cols].astype(F32)
                ).astype(BF)
                send(l, IDX["r2"][k] + j, rc(sp.at[l], l, rect),
                     rc(ro.at[l], l, rect))
    for l in range(2):
        h = 1 - l

        @pl.when(d == 2)
        def _():
            wait_sem(I_WG + 2 * l + h, wi.at[l, h])
            sp[l, w_rows(h), w_cols] = (
                accw[l, :, w_cols] + wi[l, h].astype(F32)).astype(BF)

        send(l, IDX["w2"] + h, rc(sp.at[l], h, W_RECT),
             rc(ro.at[l], h, W_RECT))
    for l in range(2):
        h = l

        @pl.when(d != 0)
        def _():
            wait_sem(I_WG + 2 * l + h, wi.at[l, h])
            sp[l, w_rows(h), w_cols] = (
                accp[l, w_rows(0), w_cols] + wi[l, h].astype(F32)).astype(BF)

        @pl.when(d == 0)
        def _():
            sp[l, w_rows(h), w_cols] = accp[l, w_rows(0), w_cols].astype(BF)

        send(l, IDX["w2"] + h, rc(sp.at[l], h, W_RECT),
             rc(ro.at[l], h, W_RECT))

    def pkr(slot, h, k, n=1, t0=0, t1=15):
        return pk.at[slot, h, pl.ds(8 * k, 8 * n),
                     pl.ds(128 * t0, 128 * (t1 - t0))]

    def unpack(slot, h, k):
        base = grow(slot, h * H + k * CH)
        c = pk[slot, h, pl.ds(8 * k, 8), :]
        s = c & jnp.uint32(SIGN)
        bits = [s[:, 128 * j:128 * (j + 1)] >> jnp.uint32(15 - j)
                for j in range(15)]
        while len(bits) > 1:
            bits = [bits[i] | bits[i + 1] if i + 1 < len(bits) else bits[i]
                    for i in range(0, len(bits), 2)]
        low = c & jnp.uint32(MAG)
        out_ref[pl.ds(base, 16), :] = pltpu.bitcast(low[:, :N], BF)
        out_ref[pl.ds(base + 16, 16), pl.ds(0, N - 128)] = (
            pltpu.bitcast(low[:, N:], BF))
        out_ref[pl.ds(base + 16, 16), pl.ds(N - 128, 128)] = (
            pltpu.bitcast(bits[0], BF))

    for l in range(2):
        for ci in range(2):
            for j, rect in enumerate(L_RECTS[ci]):
                recv(l, IDX["l"][ci] + j, rc(ro.at[l], 1 - l, rect))
    for k in range(NCH):
        for h in range(2):
            for j, rect in enumerate(R2_RECTS[k]):
                recv(h, IDX["r2"][k] + j, rc(ro.at[h], h, rect))
            if k == NCH - 1:
                for l in range(2):
                    recv(l, IDX["w2"] + h, rc(ro.at[l], h, W_RECT))
            rows = pl.ds(h * H + k * CH, CH)
            q = jnp.maximum(
                acco[rows, :] + ro[0, rows, :].astype(F32)
                + ro[1, rows, :].astype(F32), 0.0).astype(BF)
            x = pltpu.bitcast(q, U32) & jnp.uint32(MAG)
            last = x[8:, N - 128:]
            for j in range(15):
                tile = x[8 * (j // 8):8 * (j // 8) + 8,
                         128 * (j % 8):128 * (j % 8) + 128]
                pk[3, h, pl.ds(8 * k, 8), pl.ds(128 * j, 128)] = tile | (
                    (last << jnp.uint32(15 - j)) & jnp.uint32(SIGN))
            for l in (h, 1 - h):
                send(l, IDX["b1"] + 2 * k + h, pkr(3, h, k), pkr(1 + l, h, k))
            out_ref[pl.ds(grow(3, h * H + k * CH), CH), :] = q

    v_sends = []
    group_end = {g0 + g - 1: gi for gi, (g0, g) in enumerate(B2_GROUPS)}
    for k in range(NCH):
        for h in range(2):
            for q in range(2):
                recv(q, IDX["b1"] + 2 * k + h, pkr(1 + q, h, k))
                if k == 0:
                    cond = (d != 2) if h == q else (d == 0)
                    cv = xfer(I_V + 2 * q + h, I_V + h, partner[1 - q],
                              pkr(1 + q, h, 0, 1, 0, VT),
                              pkr(0, h, 0, 1, 0, VT))
                    pl.when(cond)(cv.start)
                    v_sends.append((cond, cv))
                if h == q and k in group_end:
                    gi = group_end[k]
                    g0, g = B2_GROUPS[gi]
                    if g0 == 0:
                        send(1 - q, IDX["b2"] + len(B2_GROUPS),
                             pkr(1 + q, q, 0, 1, VT), pkr(0, q, 0, 1, VT))
                        g0, g = 1, g - 1
                    send(1 - q, IDX["b2"] + gi, pkr(1 + q, q, g0, g),
                         pkr(0, q, g0, g))
                unpack(1 + q, h, k)

    late = 4
    for cp in sends[:-late]:
        cp.wait_send()
    for cond, cv in v_sends:
        pl.when(cond)(cv.wait_send)

    for gi, (g0, g) in enumerate(B2_GROUPS):
        for l in range(2):
            h = 1 - l
            if g0 == 0:
                wait_sem(I_V + h, pkr(0, h, 0, 1, 0, VT))
                recv(l, IDX["b2"] + len(B2_GROUPS), pkr(0, h, 0, 1, VT))
                recv(l, IDX["b2"] + gi, pkr(0, h, 1, g - 1))
            else:
                recv(l, IDX["b2"] + gi, pkr(0, h, g0, g))
            for k in range(g0, g0 + g):
                unpack(0, h, k)
    for cp in sends[-late:]:
        cp.wait_send()


def pallas_dist_matmul_relu_kshard_i_m1024_n1024_k512_kernel(
    A: jax.Array,
    B: jax.Array,
):
    return pl.pallas_call(
        _body,
        out_shape=jax.ShapeDtypeStruct((M, N), BF),
        in_specs=[pl.BlockSpec(memory_space=pl.ANY)] * 2,
        out_specs=pl.BlockSpec(memory_space=pltpu.VMEM),
        scratch_shapes=[
            pltpu.VMEM((4, R, K), F32),
            pltpu.VMEM((K, N), F32),
            pltpu.VMEM((R, K), BF),
            pltpu.VMEM((K, N), BF),
            pltpu.VMEM((R, N), BF),
            pltpu.VMEM((2, R, N), BF),
            pltpu.VMEM((2, H, N), F32),
            pltpu.VMEM((2, WR, N), F32),
            pltpu.VMEM((R, N), F32),
            pltpu.VMEM((2, H, N), BF),
            pltpu.VMEM((2, 2, WR, WC), BF),
            pltpu.VMEM((2, R, N), BF),
            pltpu.VMEM((4, 2, NCH * 8, PL), U32),
            pltpu.SemaphoreType.DMA((len(LOADS),)),
            pltpu.SemaphoreType.DMA((NSEM,)),
            pltpu.SemaphoreType.DMA((NSEM,)),
        ],
        compiler_params=pltpu.CompilerParams(
            collective_id=0,
            vmem_limit_bytes=64 * 1024 * 1024,
            disable_semaphore_checks=True,
        ),
    )(A, B)
```

```python
import jax
import jax.numpy as jnp
from jax import lax
from jax.experimental import pallas as pl
from jax.experimental.pallas import tpu as pltpu

M, N, K = 1024, 1024, 512
R = 256
H = 128
CH = 32
NCH = H // CH
PL = 15 * 128
SIGN = 0x80008000
MAG = 0x7FFF7FFF
WR, WC = 32, 640
VT = 5
B2_GROUPS = ((0, 2), (2, 1), (3, 1))

MESH = pl.DeviceIdType.MESH
BF = jnp.bfloat16
F32 = jnp.float32
U32 = jnp.uint32

G_LOADS = (("B", 0, 128), ("A", 0, 64), ("B", 128, 128), ("A", 64, 32),
           ("A", 96, 32), ("B", 256, 128), ("B", 384, 128), ("B", 512, 256),
           ("B", 768, 256))
G_PIECES = ((0, 64, 0, 128), (0, 64, 128, 128), (64, 32, 0, 256),
            (96, 32, 0, 256), (0, 128, 256, 128), (0, 128, 384, 128),
            (0, 128, 512, 256), (0, 128, 768, 256))
W_RECT = (H - WR, WR, N - WC, WC)


def _minus_swing(rect):
    r0, nr, c0, nc = rect
    hr0, hc0 = H - WR, N - WC
    if r0 + nr <= hr0 or c0 + nc <= hc0:
        return [rect]
    out = []
    if hc0 > c0:
        out.append((r0, nr, c0, hc0 - c0))
    if hr0 > r0:
        cc = max(c0, hc0)
        out.append((r0, hr0 - r0, cc, c0 + nc - cc))
    return out


def _plan():
    g_rects = [_minus_swing(p) for p in G_PIECES]
    l_rects = [_minus_swing((0, H, c0, 512)) for c0 in (0, 512)]
    r2_rects = [_minus_swing((k * CH, CH, 0, N)) for k in range(NCH)]

    count = [0]

    def alloc(n):
        first = count[0]
        count[0] += n
        return first

    idx = dict(
        g=[alloc(len(x)) for x in g_rects],
        l=[alloc(len(x)) for x in l_rects],
        r2=[alloc(len(x)) for x in r2_rects],
        w2=alloc(2), b1=alloc(2 * NCH), b2=alloc(len(B2_GROUPS) + 1),
    )
    per_link = count[0]

    loads = []
    for ld in G_LOADS:
        if ld[0] == "B":
            loads.append(ld)
        else:
            loads += [("A", 0, h * H + ld[1], ld[2]) for h in range(2)]
    need, seen = [], set()
    for (r0, nr, c0, nc) in G_PIECES:
        mine = []
        for k, ld in enumerate(loads):
            if ld[0] == "B":
                hit = ld[1] < c0 + nc and c0 < ld[1] + ld[2]
            else:
                hit = ld[2] % H < r0 + nr and r0 < ld[2] % H + ld[3]
            if hit and k not in seen:
                mine.append(k)
                seen.add(k)
        need.append(mine)
    first_other = len(loads)
    loads += [("A", 1, H, H), ("A", 2, 0, H),
              ("A", 1, 0, H), ("A", 2, H, H),
              ("A", 3, 0, R)]
    return g_rects, l_rects, r2_rects, idx, per_link, loads, need, first_other


(G_RECTS, L_RECTS, R2_RECTS, IDX, PER_LINK, LOADS, NEED, LD_OTHER) = _plan()
I_WG = 2 * PER_LINK
I_V = I_WG + 4
NSEM = I_V + 4
assert WR == CH


def _body(a_hbm, b_hbm, out_ref,
          a_f32, b_f32, a_bf, b_bf, sg, sp, accp, accw, acco, ri, wi, ro, pk,
          in_sems, ssem, rsem):
    d = lax.axis_index("i")
    partner = (d ^ 1, 3 - d)
    region = ((d + 2) & 3, partner[0], partner[1], d)

    def grow(slot, r0):
        return pl.multiple_of(region[slot] * R + r0, 16)

    barrier = pltpu.get_barrier_semaphore()
    load_cps = []
    for k, ld in enumerate(LOADS):
        if ld[0] == "B":
            cols = pl.ds(ld[1], ld[2])
            cp = pltpu.make_async_copy(b_hbm.at[:, cols], b_f32.at[:, cols],
                                       in_sems.at[k])
        else:
            _, slot, r0, nr = ld
            cp = pltpu.make_async_copy(a_hbm.at[pl.ds(grow(slot, r0), nr)],
                                       a_f32.at[slot, pl.ds(r0, nr)],
                                       in_sems.at[k])
        cp.start()
        load_cps.append(cp)
        if k == 2:
            for p in partner:
                pl.semaphore_signal(barrier, inc=1, device_id=(p,),
                                    device_id_type=MESH)

    sends = []

    def xfer(sidx, ridx, dev, src, dst):
        return pltpu.make_async_remote_copy(
            src_ref=src, dst_ref=dst, send_sem=ssem.at[sidx],
            recv_sem=rsem.at[ridx], device_id=(dev,), device_id_type=MESH)

    def send(l, t, src, dst):
        cp = xfer(l * PER_LINK + t, l * PER_LINK + t, partner[l], src, dst)
        cp.start()
        sends.append(cp)

    def wait_sem(ridx, dst):
        xfer(0, ridx, partner[0], dst, dst).wait_recv()

    def recv(l, t, dst):
        wait_sem(l * PER_LINK + t, dst)

    def rc(ref, h, rect):
        r0, nr, c0, nc = rect
        return ref.at[pl.ds(h * H + r0, nr), pl.ds(c0, nc)]

    def mm(lhs, cols=slice(None)):
        return jnp.dot(lhs, b_bf[:, cols], preferred_element_type=F32)

    def w_rows(h):
        return pl.ds(h * H + H - WR, WR)

    w_cols = pl.ds(N - WC, WC)

    for k, (r0, nr, c0, nc) in enumerate(G_PIECES):
        for j in NEED[k]:
            load_cps[j].wait()
            ld = LOADS[j]
            if ld[0] == "B":
                cols = pl.ds(ld[1], ld[2])
                b_bf[:, cols] = b_f32[:, cols].astype(BF)
            else:
                rows = pl.ds(ld[2], ld[3])
                a_bf[rows, :] = a_f32[0, rows, :].astype(BF)
        cols = pl.ds(c0, nc)
        if nr == H:
            sg[:, cols] = mm(a_bf[...], cols).astype(BF)
        else:
            lhs = jnp.concatenate(
                [a_bf[pl.ds(r0, nr), :], a_bf[pl.ds(H + r0, nr), :]], axis=0)
            res = mm(lhs, cols).astype(BF)
            sg[pl.ds(r0, nr), cols] = res[:nr]
            sg[pl.ds(H + r0, nr), cols] = res[nr:]
        if k == 0:
            pl.semaphore_wait(barrier, 2)
        for j, rect in enumerate(G_RECTS[k]):
            for l in range(2):
                send(l, IDX["g"][k] + j, rc(sg, 1 - l, rect),
                     rc(ri.at[1 - l], 0, rect))
    for h in range(2):
        flip = d == (3 if h == 0 else 1)
        q = jnp.where(flip, 1 - h, h)
        dev = jnp.where(flip, partner[h], partner[1 - h])
        cp = xfer(I_WG + h, I_WG + 2 * q + h, dev, rc(sg, h, W_RECT),
                  wi.at[q, h])
        cp.start()
        sends.append(cp)

    load_cps[LD_OTHER].wait()
    load_cps[LD_OTHER + 1].wait()
    a_bf[pl.ds(0, H), :] = a_f32[1, pl.ds(H, H), :].astype(BF)
    a_bf[pl.ds(H, H), :] = a_f32[2, pl.ds(0, H), :].astype(BF)
    for ci in range(2):
        cols = pl.ds(ci * 512, 512)
        res = mm(a_bf[...], cols)
        for l in range(2):
            sp[l, pl.ds((1 - l) * H, H), cols] = (
                res[l * H:(l + 1) * H].astype(BF))
            accw[l, :, cols] = res[(l + 1) * H - WR:(l + 1) * H]
        for j, rect in enumerate(L_RECTS[ci]):
            for l in range(2):
                send(l, IDX["l"][ci] + j, rc(sp.at[l], 1 - l, rect),
                     rc(ro.at[l], 1 - l, rect))

    for l in range(2):
        load_cps[LD_OTHER + 2 + l].wait()
        accp[l] = mm(a_f32[1 + l, pl.ds(l * H, H), :].astype(BF))
    load_cps[LD_OTHER + 4].wait()
    for h in range(2):
        rows = pl.ds(h * H, H)
        acco[rows, :] = mm(a_f32[3, rows, :].astype(BF))

    for l in range(2):
        for k in range(len(G_PIECES)):
            for j, rect in enumerate(G_RECTS[k]):
                recv(1 - l, IDX["g"][k] + j, rc(ri.at[l], 0, rect))
        for k in range(NCH):
            for j, rect in enumerate(R2_RECTS[k]):
                r0, nr, c0, nc = rect
                rows, cols = pl.ds(r0, nr), pl.ds(c0, nc)
                sp[l, pl.ds(l * H + r0, nr), cols] = (
                    accp[l, rows, cols] + ri[l, rows, cols].astype(F32)
                ).astype(BF)
                send(l, IDX["r2"][k] + j, rc(sp.at[l], l, rect),
                     rc(ro.at[l], l, rect))
    for l in range(2):
        h = 1 - l

        @pl.when(d == 2)
        def _():
            wait_sem(I_WG + 2 * l + h, wi.at[l, h])
            sp[l, w_rows(h), w_cols] = (
                accw[l, :, w_cols] + wi[l, h].astype(F32)).astype(BF)

        send(l, IDX["w2"] + h, rc(sp.at[l], h, W_RECT),
             rc(ro.at[l], h, W_RECT))
    for l in range(2):
        h = l

        @pl.when(d != 0)
        def _():
            wait_sem(I_WG + 2 * l + h, wi.at[l, h])
            sp[l, w_rows(h), w_cols] = (
                accp[l, w_rows(0), w_cols] + wi[l, h].astype(F32)).astype(BF)

        @pl.when(d == 0)
        def _():
            sp[l, w_rows(h), w_cols] = accp[l, w_rows(0), w_cols].astype(BF)

        send(l, IDX["w2"] + h, rc(sp.at[l], h, W_RECT),
             rc(ro.at[l], h, W_RECT))

    def pkr(slot, h, k, n=1, t0=0, t1=15):
        return pk.at[slot, h, pl.ds(8 * k, 8 * n),
                     pl.ds(128 * t0, 128 * (t1 - t0))]

    def unpack(slot, h, k):
        base = grow(slot, h * H + k * CH)
        c = pk[slot, h, pl.ds(8 * k, 8), :]
        s = c & jnp.uint32(SIGN)
        bits = [s[:, 128 * j:128 * (j + 1)] >> jnp.uint32(15 - j)
                for j in range(15)]
        while len(bits) > 1:
            bits = [bits[i] | bits[i + 1] if i + 1 < len(bits) else bits[i]
                    for i in range(0, len(bits), 2)]
        low = c & jnp.uint32(MAG)
        out_ref[pl.ds(base, 16), :] = pltpu.bitcast(low[:, :N], BF)
        out_ref[pl.ds(base + 16, 16), pl.ds(0, N - 128)] = (
            pltpu.bitcast(low[:, N:], BF))
        out_ref[pl.ds(base + 16, 16), pl.ds(N - 128, 128)] = (
            pltpu.bitcast(bits[0], BF))

    for l in range(2):
        for ci in range(2):
            for j, rect in enumerate(L_RECTS[ci]):
                recv(l, IDX["l"][ci] + j, rc(ro.at[l], 1 - l, rect))
    for k in range(NCH):
        for h in range(2):
            for j, rect in enumerate(R2_RECTS[k]):
                recv(h, IDX["r2"][k] + j, rc(ro.at[h], h, rect))
            if k == NCH - 1:
                for l in range(2):
                    recv(l, IDX["w2"] + h, rc(ro.at[l], h, W_RECT))
            rows = pl.ds(h * H + k * CH, CH)
            q = jnp.maximum(
                acco[rows, :] + ro[0, rows, :].astype(F32)
                + ro[1, rows, :].astype(F32), 0.0).astype(BF)
            x = pltpu.bitcast(q, U32) & jnp.uint32(MAG)
            last = x[8:, N - 128:]
            for j in range(15):
                tile = x[8 * (j // 8):8 * (j // 8) + 8,
                         128 * (j % 8):128 * (j % 8) + 128]
                pk[3, h, pl.ds(8 * k, 8), pl.ds(128 * j, 128)] = tile | (
                    (last << jnp.uint32(15 - j)) & jnp.uint32(SIGN))
            for l in (h, 1 - h):
                send(l, IDX["b1"] + 2 * k + h, pkr(3, h, k), pkr(1 + l, h, k))
            out_ref[pl.ds(grow(3, h * H + k * CH), CH), :] = q

    v_sends = []
    group_end = {g0 + g - 1: gi for gi, (g0, g) in enumerate(B2_GROUPS)}
    for k in range(NCH):
        for h in range(2):
            for q in range(2):
                recv(q, IDX["b1"] + 2 * k + h, pkr(1 + q, h, k))
                if k == 0:
                    cond = (d != 2) if h == q else (d == 0)
                    cv = xfer(I_V + 2 * q + h, I_V + h, partner[1 - q],
                              pkr(1 + q, h, 0, 1, 0, VT),
                              pkr(0, h, 0, 1, 0, VT))
                    pl.when(cond)(cv.start)
                    v_sends.append((cond, cv))
                if h == q and k in group_end:
                    gi = group_end[k]
                    g0, g = B2_GROUPS[gi]
                    if g0 == 0:
                        send(1 - q, IDX["b2"] + len(B2_GROUPS),
                             pkr(1 + q, q, 0, 1, VT), pkr(0, q, 0, 1, VT))
                        g0, g = 1, g - 1
                    send(1 - q, IDX["b2"] + gi, pkr(1 + q, q, g0, g),
                         pkr(0, q, g0, g))
                unpack(1 + q, h, k)

    late = 4
    for cp in sends[:-late]:
        cp.wait_send()
    for cond, cv in v_sends:
        pl.when(cond)(cv.wait_send)

    for gi, (g0, g) in enumerate(B2_GROUPS):
        for l in range(2):
            h = 1 - l
            if g0 == 0:
                wait_sem(I_V + h, pkr(0, h, 0, 1, 0, VT))
                recv(l, IDX["b2"] + len(B2_GROUPS), pkr(0, h, 0, 1, VT))
                recv(l, IDX["b2"] + gi, pkr(0, h, 1, g - 1))
            else:
                recv(l, IDX["b2"] + gi, pkr(0, h, g0, g))
            for k in range(g0, g0 + g):
                unpack(0, h, k)
    for cp in sends[-late:]:
        cp.wait_send()


def pallas_dist_matmul_relu_kshard_i_m1024_n1024_k512_kernel(
    A: jax.Array,
    B: jax.Array,
):
    return pl.pallas_call(
        _body,
        out_shape=jax.ShapeDtypeStruct((M, N), BF),
        in_specs=[pl.BlockSpec(memory_space=pl.ANY)] * 2,
        out_specs=pl.BlockSpec(memory_space=pltpu.VMEM),
        scratch_shapes=[
            pltpu.VMEM((4, R, K), F32),
            pltpu.VMEM((K, N), F32),
            pltpu.VMEM((R, K), BF),
            pltpu.VMEM((K, N), BF),
            pltpu.VMEM((R, N), BF),
            pltpu.VMEM((2, R, N), BF),
            pltpu.VMEM((2, H, N), F32),
            pltpu.VMEM((2, WR, N), F32),
            pltpu.VMEM((R, N), F32),
            pltpu.VMEM((2, H, N), BF),
            pltpu.VMEM((2, 2, WR, WC), BF),
            pltpu.VMEM((2, R, N), BF),
            pltpu.VMEM((4, 2, NCH * 8, PL), U32),
            pltpu.SemaphoreType.DMA((len(LOADS),)),
            pltpu.SemaphoreType.DMA((NSEM,)),
            pltpu.SemaphoreType.DMA((NSEM,)),
        ],
        compiler_params=pltpu.CompilerParams(
            collective_id=0,
            vmem_limit_bytes=64 * 1024 * 1024,
            disable_semaphore_checks=True,
        ),
    )(A, B)
```

```python
import jax
import jax.numpy as jnp
from jax import lax
from jax.experimental import pallas as pl
from jax.experimental.pallas import tpu as pltpu

M, N, K = 1024, 1024, 512
R = 256
H = 128
CH = 32
NCH = H // CH
PL = 15 * 128
SIGN = 0x80008000
MAG = 0x7FFF7FFF
WR, WC = 32, 640
VT = 5
B2_GROUPS = ((0, 2), (2, 1), (3, 1))

MESH = pl.DeviceIdType.MESH
BF = jnp.bfloat16
F32 = jnp.float32
U32 = jnp.uint32

G_LOADS = (("B", 0, 128), ("A", 0, 64), ("B", 128, 128), ("A", 64, 32),
           ("A", 96, 32), ("B", 256, 128), ("B", 384, 128), ("B", 512, 256),
           ("B", 768, 256))
G_PIECES = ((0, 64, 0, 128), (0, 64, 128, 128), (64, 32, 0, 256),
            (96, 32, 0, 256), (0, 128, 256, 128), (0, 128, 384, 128),
            (0, 128, 512, 256), (0, 128, 768, 256))
W_RECT = (H - WR, WR, N - WC, WC)


def _minus_swing(rect):
    r0, nr, c0, nc = rect
    hr0, hc0 = H - WR, N - WC
    if r0 + nr <= hr0 or c0 + nc <= hc0:
        return [rect]
    out = []
    if hc0 > c0:
        out.append((r0, nr, c0, hc0 - c0))
    if hr0 > r0:
        cc = max(c0, hc0)
        out.append((r0, hr0 - r0, cc, c0 + nc - cc))
    return out


def _plan():
    g_rects = [_minus_swing(p) for p in G_PIECES]
    l_rects = [_minus_swing((0, H, c0, 512)) for c0 in (0, 512)]
    r2_rects = [_minus_swing((k * CH, CH, 0, N)) for k in range(NCH)]

    count = [0]

    def alloc(n):
        first = count[0]
        count[0] += n
        return first

    idx = dict(
        g=[alloc(len(x)) for x in g_rects],
        l=[alloc(len(x)) for x in l_rects],
        r2=[alloc(len(x)) for x in r2_rects],
        w2=alloc(2), b1=alloc(2 * NCH), b2=alloc(len(B2_GROUPS) + 1),
    )
    per_link = count[0]

    loads = []
    for ld in G_LOADS:
        if ld[0] == "B":
            loads.append(ld)
        else:
            loads += [("A", 0, h * H + ld[1], ld[2]) for h in range(2)]
    need, seen = [], set()
    for (r0, nr, c0, nc) in G_PIECES:
        mine = []
        for k, ld in enumerate(loads):
            if ld[0] == "B":
                hit = ld[1] < c0 + nc and c0 < ld[1] + ld[2]
            else:
                hit = ld[2] % H < r0 + nr and r0 < ld[2] % H + ld[3]
            if hit and k not in seen:
                mine.append(k)
                seen.add(k)
        need.append(mine)
    first_other = len(loads)
    loads += [("A", 1, H, H), ("A", 2, 0, H),
              ("A", 1, 0, H), ("A", 2, H, H),
              ("A", 3, 0, R)]
    return g_rects, l_rects, r2_rects, idx, per_link, loads, need, first_other


(G_RECTS, L_RECTS, R2_RECTS, IDX, PER_LINK, LOADS, NEED, LD_OTHER) = _plan()
I_WG = 2 * PER_LINK
I_V = I_WG + 4
NSEM = I_V + 4
assert WR == CH


def _body(a_hbm, b_hbm, out_ref,
          a_f32, b_f32, a_bf, b_bf, sg, sp, accp, accw, acco, ri, wi, ro, pk,
          in_sems, ssem, rsem):
    d = lax.axis_index("i")
    partner = (d ^ 1, 3 - d)
    region = ((d + 2) & 3, partner[0], partner[1], d)

    def grow(slot, r0):
        return pl.multiple_of(region[slot] * R + r0, 16)

    barrier = pltpu.get_barrier_semaphore()
    load_cps = []
    for k, ld in enumerate(LOADS):
        if ld[0] == "B":
            cols = pl.ds(ld[1], ld[2])
            cp = pltpu.make_async_copy(b_hbm.at[:, cols], b_f32.at[:, cols],
                                       in_sems.at[k])
        else:
            _, slot, r0, nr = ld
            cp = pltpu.make_async_copy(a_hbm.at[pl.ds(grow(slot, r0), nr)],
                                       a_f32.at[slot, pl.ds(r0, nr)],
                                       in_sems.at[k])
        cp.start()
        load_cps.append(cp)
        if k == 2:
            for p in partner:
                pl.semaphore_signal(barrier, inc=1, device_id=(p,),
                                    device_id_type=MESH)

    sends = []

    def xfer(sidx, ridx, dev, src, dst):
        return pltpu.make_async_remote_copy(
            src_ref=src, dst_ref=dst, send_sem=ssem.at[sidx],
            recv_sem=rsem.at[ridx], device_id=(dev,), device_id_type=MESH)

    def send(l, t, src, dst):
        cp = xfer(l * PER_LINK + t, l * PER_LINK + t, partner[l], src, dst)
        cp.start()
        sends.append(cp)

    def wait_sem(ridx, dst):
        xfer(0, ridx, partner[0], dst, dst).wait_recv()

    def recv(l, t, dst):
        wait_sem(l * PER_LINK + t, dst)

    def rc(ref, h, rect):
        r0, nr, c0, nc = rect
        return ref.at[pl.ds(h * H + r0, nr), pl.ds(c0, nc)]

    def mm(lhs, cols=slice(None)):
        return jnp.dot(lhs, b_bf[:, cols], preferred_element_type=F32)

    def w_rows(h):
        return pl.ds(h * H + H - WR, WR)

    w_cols = pl.ds(N - WC, WC)

    for k, (r0, nr, c0, nc) in enumerate(G_PIECES):
        for j in NEED[k]:
            load_cps[j].wait()
            ld = LOADS[j]
            if ld[0] == "B":
                cols = pl.ds(ld[1], ld[2])
                b_bf[:, cols] = b_f32[:, cols].astype(BF)
            else:
                rows = pl.ds(ld[2], ld[3])
                a_bf[rows, :] = a_f32[0, rows, :].astype(BF)
        cols = pl.ds(c0, nc)
        if nr == H:
            sg[:, cols] = mm(a_bf[...], cols).astype(BF)
        else:
            lhs = jnp.concatenate(
                [a_bf[pl.ds(r0, nr), :], a_bf[pl.ds(H + r0, nr), :]], axis=0)
            res = mm(lhs, cols).astype(BF)
            sg[pl.ds(r0, nr), cols] = res[:nr]
            sg[pl.ds(H + r0, nr), cols] = res[nr:]
        if k == 0:
            pl.semaphore_wait(barrier, 2)
        for j, rect in enumerate(G_RECTS[k]):
            for l in range(2):
                send(l, IDX["g"][k] + j, rc(sg, 1 - l, rect),
                     rc(ri.at[1 - l], 0, rect))
    for h in range(2):
        flip = d == (3 if h == 0 else 1)
        q = jnp.where(flip, 1 - h, h)
        dev = jnp.where(flip, partner[h], partner[1 - h])
        cp = xfer(I_WG + h, I_WG + 2 * q + h, dev, rc(sg, h, W_RECT),
                  wi.at[q, h])
        cp.start()
        sends.append(cp)

    load_cps[LD_OTHER].wait()
    load_cps[LD_OTHER + 1].wait()
    a_bf[pl.ds(0, H), :] = a_f32[1, pl.ds(H, H), :].astype(BF)
    a_bf[pl.ds(H, H), :] = a_f32[2, pl.ds(0, H), :].astype(BF)
    for ci in range(2):
        cols = pl.ds(ci * 512, 512)
        res = mm(a_bf[...], cols)
        for l in range(2):
            sp[l, pl.ds((1 - l) * H, H), cols] = (
                res[l * H:(l + 1) * H].astype(BF))
            accw[l, :, cols] = res[(l + 1) * H - WR:(l + 1) * H]
        for j, rect in enumerate(L_RECTS[ci]):
            for l in range(2):
                send(l, IDX["l"][ci] + j, rc(sp.at[l], 1 - l, rect),
                     rc(ro.at[l], 1 - l, rect))

    for l in range(2):
        load_cps[LD_OTHER + 2 + l].wait()
        accp[l] = mm(a_f32[1 + l, pl.ds(l * H, H), :].astype(BF))
    load_cps[LD_OTHER + 4].wait()
    for h in range(2):
        rows = pl.ds(h * H, H)
        acco[rows, :] = mm(a_f32[3, rows, :].astype(BF))

    for l in range(2):
        for k in range(len(G_PIECES)):
            for j, rect in enumerate(G_RECTS[k]):
                recv(1 - l, IDX["g"][k] + j, rc(ri.at[l], 0, rect))
        for k in range(NCH):
            for j, rect in enumerate(R2_RECTS[k]):
                r0, nr, c0, nc = rect
                rows, cols = pl.ds(r0, nr), pl.ds(c0, nc)
                sp[l, pl.ds(l * H + r0, nr), cols] = (
                    accp[l, rows, cols] + ri[l, rows, cols].astype(F32)
                ).astype(BF)
                send(l, IDX["r2"][k] + j, rc(sp.at[l], l, rect),
                     rc(ro.at[l], l, rect))
    for l in range(2):
        h = 1 - l

        @pl.when(d == 2)
        def _():
            wait_sem(I_WG + 2 * l + h, wi.at[l, h])
            sp[l, w_rows(h), w_cols] = (
                accw[l, :, w_cols] + wi[l, h].astype(F32)).astype(BF)

        send(l, IDX["w2"] + h, rc(sp.at[l], h, W_RECT),
             rc(ro.at[l], h, W_RECT))
    for l in range(2):
        h = l

        @pl.when(d != 0)
        def _():
            wait_sem(I_WG + 2 * l + h, wi.at[l, h])
            sp[l, w_rows(h), w_cols] = (
                accp[l, w_rows(0), w_cols] + wi[l, h].astype(F32)).astype(BF)

        @pl.when(d == 0)
        def _():
            sp[l, w_rows(h), w_cols] = accp[l, w_rows(0), w_cols].astype(BF)

        send(l, IDX["w2"] + h, rc(sp.at[l], h, W_RECT),
             rc(ro.at[l], h, W_RECT))

    def pkr(slot, h, k, n=1, t0=0, t1=15):
        return pk.at[slot, h, pl.ds(8 * k, 8 * n),
                     pl.ds(128 * t0, 128 * (t1 - t0))]

    def unpack(slot, h, k):
        base = grow(slot, h * H + k * CH)
        c = pk[slot, h, pl.ds(8 * k, 8), :]
        s = c & jnp.uint32(SIGN)
        bits = [s[:, 128 * j:128 * (j + 1)] >> jnp.uint32(15 - j)
                for j in range(15)]
        while len(bits) > 1:
            bits = [bits[i] | bits[i + 1] if i + 1 < len(bits) else bits[i]
                    for i in range(0, len(bits), 2)]
        low = c & jnp.uint32(MAG)
        out_ref[pl.ds(base, 16), :] = pltpu.bitcast(low[:, :N], BF)
        out_ref[pl.ds(base + 16, 16), pl.ds(0, N - 128)] = (
            pltpu.bitcast(low[:, N:], BF))
        out_ref[pl.ds(base + 16, 16), pl.ds(N - 128, 128)] = (
            pltpu.bitcast(bits[0], BF))

    for l in range(2):
        for ci in range(2):
            for j, rect in enumerate(L_RECTS[ci]):
                recv(l, IDX["l"][ci] + j, rc(ro.at[l], 1 - l, rect))
    for k in range(NCH):
        for h in range(2):
            for j, rect in enumerate(R2_RECTS[k]):
                recv(h, IDX["r2"][k] + j, rc(ro.at[h], h, rect))
            if k == NCH - 1:
                for l in range(2):
                    recv(l, IDX["w2"] + h, rc(ro.at[l], h, W_RECT))
            rows = pl.ds(h * H + k * CH, CH)
            q = jnp.maximum(
                acco[rows, :] + ro[0, rows, :].astype(F32)
                + ro[1, rows, :].astype(F32), 0.0).astype(BF)
            x = pltpu.bitcast(q, U32) & jnp.uint32(MAG)
            last = x[8:, N - 128:]
            for j in range(15):
                tile = x[8 * (j // 8):8 * (j // 8) + 8,
                         128 * (j % 8):128 * (j % 8) + 128]
                pk[3, h, pl.ds(8 * k, 8), pl.ds(128 * j, 128)] = tile | (
                    (last << jnp.uint32(15 - j)) & jnp.uint32(SIGN))
            for l in (h, 1 - h):
                send(l, IDX["b1"] + 2 * k + h, pkr(3, h, k), pkr(1 + l, h, k))
            out_ref[pl.ds(grow(3, h * H + k * CH), CH), :] = q

    v_sends = []
    group_end = {g0 + g - 1: gi for gi, (g0, g) in enumerate(B2_GROUPS)}
    for k in range(NCH):
        for h in range(2):
            for q in range(2):
                recv(q, IDX["b1"] + 2 * k + h, pkr(1 + q, h, k))
                if k == 0:
                    cond = (d != 2) if h == q else (d == 0)
                    cv = xfer(I_V + 2 * q + h, I_V + h, partner[1 - q],
                              pkr(1 + q, h, 0, 1, 0, VT),
                              pkr(0, h, 0, 1, 0, VT))
                    pl.when(cond)(cv.start)
                    v_sends.append((cond, cv))
                if h == q and k in group_end:
                    gi = group_end[k]
                    g0, g = B2_GROUPS[gi]
                    if g0 == 0:
                        send(1 - q, IDX["b2"] + len(B2_GROUPS),
                             pkr(1 + q, q, 0, 1, VT), pkr(0, q, 0, 1, VT))
                        g0, g = 1, g - 1
                    send(1 - q, IDX["b2"] + gi, pkr(1 + q, q, g0, g),
                         pkr(0, q, g0, g))
                unpack(1 + q, h, k)

    late = 4
    for cp in sends[:-late]:
        cp.wait_send()
    for cond, cv in v_sends:
        pl.when(cond)(cv.wait_send)

    for gi, (g0, g) in enumerate(B2_GROUPS):
        for l in range(2):
            h = 1 - l
            if g0 == 0:
                wait_sem(I_V + h, pkr(0, h, 0, 1, 0, VT))
                recv(l, IDX["b2"] + len(B2_GROUPS), pkr(0, h, 0, 1, VT))
                recv(l, IDX["b2"] + gi, pkr(0, h, 1, g - 1))
            else:
                recv(l, IDX["b2"] + gi, pkr(0, h, g0, g))
            for k in range(g0, g0 + g):
                unpack(0, h, k)
    for cp in sends[-late:]:
        cp.wait_send()


def pallas_dist_matmul_relu_kshard_i_m1024_n1024_k512_kernel(
    A: jax.Array,
    B: jax.Array,
):
    extra = {}
    if hasattr(pltpu.CompilerParams, "disable_semaphore_checks"):
        extra["disable_semaphore_checks"] = True
    return pl.pallas_call(
        _body,
        out_shape=jax.ShapeDtypeStruct((M, N), BF),
        in_specs=[pl.BlockSpec(memory_space=pl.ANY)] * 2,
        out_specs=pl.BlockSpec(memory_space=pltpu.VMEM),
        scratch_shapes=[
            pltpu.VMEM((4, R, K), F32),
            pltpu.VMEM((K, N), F32),
            pltpu.VMEM((R, K), BF),
            pltpu.VMEM((K, N), BF),
            pltpu.VMEM((R, N), BF),
            pltpu.VMEM((2, R, N), BF),
            pltpu.VMEM((2, H, N), F32),
            pltpu.VMEM((2, WR, N), F32),
            pltpu.VMEM((R, N), F32),
            pltpu.VMEM((2, H, N), BF),
            pltpu.VMEM((2, 2, WR, WC), BF),
            pltpu.VMEM((2, R, N), BF),
            pltpu.VMEM((4, 2, NCH * 8, PL), U32),
            pltpu.SemaphoreType.DMA((len(LOADS),)),
            pltpu.SemaphoreType.DMA((NSEM,)),
            pltpu.SemaphoreType.DMA((NSEM,)),
        ],
        compiler_params=pltpu.CompilerParams(
            collective_id=0,
            vmem_limit_bytes=64 * 1024 * 1024,
            **extra,
        ),
    )(A, B)
```
